```python
import numpy as np

kernel_name = "dist_f_of_ar_i_m4096_n1024"

def setup_inputs():
    t = np.random.randn(16384, 1024).astype(np.float32)
    return {"t": t}

def reference(t: np.ndarray) -> np.ndarray:
    s = t.reshape(4, 4096, 1024).sum(axis=0)
    r = np.maximum(s, 0.0)
    return np.tanh(s) * s * s + r * r * r
```

```python
import jax
import jax.numpy as jnp
from jax import lax
from jax.experimental import pallas as pl
from jax.experimental.pallas import tpu as pltpu

M, N = 4096, 1024
BLK = M // 8
STEP = 16

P1 = (16, 48, 192, 256, 512)
P2 = (256, 256)
P4 = (512, 320, 128, 48, 16)


def _pieces(sizes):
    out, start = [], 0
    for size in sizes:
        out.append((start, size))
        start += size
    return out


def _rows(start, size, fn):
    if size == STEP:
        fn(pl.ds(start, STEP))
        return

    def step(i, carry):
        fn(pl.ds(pl.multiple_of(start + i * STEP, STEP), STEP))
        return carry

    lax.fori_loop(0, size // STEP, step, 0)


def _body(
    t_hbm, out_hbm,
    x, send1, recv1, send2, recv2, own, other, res,
    load_sem, store_sem, send_sem, recv_sem,
):
    me = lax.axis_index("i")
    cx = me >> 1
    cy = (me ^ cx) & 1
    peer_y = me ^ 1
    peer_x = me ^ 3
    halves = (0, 1)
    a = (cy, cx)
    b = (cx, cy)
    peer_a = (peer_y, peer_x)
    peer_b = (peer_x, peer_y)

    def block(h, far_a, far_b):
        row = h * 4 * BLK + (a[h] ^ far_a) * 2 * BLK + (b[h] ^ far_b) * BLK
        return pl.multiple_of(row, BLK)

    x_blocks = ((1, 1), (1, 0), (0, 1), (0, 0))
    res_blocks = ((0, 0), (0, 1), (1, 0), (1, 1))

    counters = {"load": 0, "store": 0, "remote": 0}

    def next_id(kind):
        counters[kind] += 1
        return counters[kind] - 1

    def load(h, start, size):
        src = block(h, *x_blocks[start // BLK]) + start % BLK
        return pltpu.make_async_copy(
            t_hbm.at[pl.ds(src, size)],
            x.at[h, pl.ds(start, size)],
            load_sem.at[next_id("load")],
        )

    def store(h, start, size):
        dst = block(h, *res_blocks[start // BLK]) + start % BLK
        return pltpu.make_async_copy(
            res.at[h, pl.ds(start, size)],
            out_hbm.at[pl.ds(dst, size)],
            store_sem.at[next_id("store")],
        )

    def remote(src, dst, peer):
        k = next_id("remote")
        return pltpu.make_async_remote_copy(
            src, dst, send_sem.at[k], recv_sem.at[k],
            device_id=(peer,), device_id_type=pl.DeviceIdType.MESH,
        )

    p1, p2, p4 = _pieces(P1), _pieces(P2), _pieces(P4)
    rest = [(2 * BLK, BLK), (3 * BLK, BLK)]
    loads = [[load(h, s, n) for h in halves] for s, n in p1 + rest]
    c1 = [
        [remote(send1.at[h, pl.ds(s, n)], recv1.at[h, pl.ds(s, n)], peer_a[h])
         for h in halves]
        for s, n in p1
    ]
    c2 = [
        [remote(send2.at[h, pl.ds(s, n)], recv2.at[h, pl.ds(s, n)], peer_b[h])
         for h in halves]
        for s, n in p2
    ]
    c3 = [
        [remote(own.at[h, pl.ds(s, n)], own.at[h, pl.ds(BLK + s, n)], peer_b[h])
         for h in halves]
        for s, n in p2
    ]
    c4 = [
        [remote(own.at[h, pl.ds(s, n)], other.at[h, pl.ds(s, n)], peer_a[h])
         for h in halves]
        for s, n in p4
    ]
    stores = []

    def write_out(h, start, size):
        copy = store(h, start, size)
        copy.start()
        stores.append(copy)

    barrier = pltpu.get_barrier_semaphore()
    for peer in (peer_y, peer_x):
        pl.semaphore_signal(
            barrier, inc=1, device_id=(peer,), device_id_type=pl.DeviceIdType.MESH
        )
    for pair in loads:
        for copy in pair:
            copy.start()

    for k, (s, n) in enumerate(p1):
        for h in halves:
            loads[k][h].wait()

            def pack(r, h=h):
                send1[h, r, :] = x[h, r, :].astype(jnp.bfloat16)

            _rows(s, n, pack)
            if k > 0:
                c1[k][h].start()
        if k == 0:
            pl.semaphore_wait(barrier, 2)
            for h in halves:
                c1[k][h].start()

    landed = [0]

    def wait_c1(upto):
        while landed[0] < len(p1) and p1[landed[0]][0] < upto:
            for h in halves:
                c1[landed[0]][h].wait_recv()
            landed[0] += 1

    for h in halves:
        loads[len(p1)][h].wait()
    for k, (s, n) in enumerate(p2):
        wait_c1(s + n)
        for h in halves:

            def add(r, h=h):
                mine = x.at[h, pl.ds(2 * BLK, BLK)][r, :]
                pair = mine + recv1[h, r, :].astype(jnp.float32)
                send2[h, r, :] = pair.astype(jnp.bfloat16)

            _rows(s, n, add)
            c2[k][h].start()

    for h in halves:
        loads[len(p1) + 1][h].wait()
    wait_c1(2 * BLK)
    for k, (s, n) in enumerate(p2):
        for h in halves:
            c2[k][h].wait_recv()

            def finish(r, h=h):
                mine = x.at[h, pl.ds(3 * BLK, BLK)][r, :]
                near = recv1.at[h, pl.ds(BLK, BLK)][r, :].astype(jnp.float32)
                v = (mine + near) + recv2[h, r, :].astype(jnp.float32)
                pos = jnp.maximum(v, 0.0)
                g = (jnp.tanh(v) * v * v + pos * pos * pos).astype(jnp.bfloat16)
                own[h, r, :] = g
                res[h, r, :] = g.astype(jnp.float32)

            _rows(s, n, finish)
            c3[k][h].start()

    arrived = [0]

    def wait_c3(upto):
        while arrived[0] < len(p2) and BLK + p2[arrived[0]][0] < upto:
            for h in halves:
                c3[arrived[0]][h].wait_recv()
            arrived[0] += 1

    for k, (s, n) in enumerate(p4):
        wait_c3(s + n)
        for h in halves:
            c4[k][h].start()
        if k == 0:
            for h in halves:
                write_out(h, 0, BLK)

    for h in halves:

        def unpack_own(r, h=h):
            res[h, r, :] = own[h, r, :].astype(jnp.float32)

        _rows(BLK, BLK, unpack_own)
        write_out(h, BLK, BLK)

    for group in (c1, c2, c3):
        for pair in group:
            for copy in pair:
                copy.wait_send()

    for k, (s, n) in enumerate(p4):
        for h in halves:
            c4[k][h].wait_recv()

            def unpack_other(r, h=h):
                far = res.at[h, pl.ds(2 * BLK, 2 * BLK)]
                far[r, :] = other[h, r, :].astype(jnp.float32)

            _rows(s, n, unpack_other)
            write_out(h, 2 * BLK + s, n)

    for pair in c4:
        for copy in pair:
            copy.wait_send()
    for copy in stores:
        copy.wait()


def pallas_dist_f_of_ar_i_m4096_n1024_kernel(t: jax.Array):
    assert t.shape == (M, N)
    n_remote = 2 * (len(P1) + 2 * len(P2) + len(P4))
    return pl.pallas_call(
        _body,
        out_shape=jax.ShapeDtypeStruct((M, N), jnp.float32),
        in_specs=[pl.BlockSpec(memory_space=pl.ANY)],
        out_specs=pl.BlockSpec(memory_space=pl.ANY),
        scratch_shapes=[
            pltpu.VMEM((2, 4 * BLK, N), jnp.float32),
            pltpu.VMEM((2, 2 * BLK, N), jnp.bfloat16),
            pltpu.VMEM((2, 2 * BLK, N), jnp.bfloat16),
            pltpu.VMEM((2, BLK, N), jnp.bfloat16),
            pltpu.VMEM((2, BLK, N), jnp.bfloat16),
            pltpu.VMEM((2, 2 * BLK, N), jnp.bfloat16),
            pltpu.VMEM((2, 2 * BLK, N), jnp.bfloat16),
            pltpu.VMEM((2, 4 * BLK, N), jnp.float32),
            pltpu.SemaphoreType.DMA((2 * (len(P1) + 2),)),
            pltpu.SemaphoreType.DMA((2 * (len(P4) + 2),)),
            pltpu.SemaphoreType.DMA((n_remote,)),
            pltpu.SemaphoreType.DMA((n_remote,)),
        ],
        compiler_params=pltpu.CompilerParams(
            collective_id=0, vmem_limit_bytes=64 * 1024 * 1024
        ),
    )(t)
```

```python
import jax
import jax.numpy as jnp
from jax import lax
from jax.experimental import pallas as pl
from jax.experimental.pallas import tpu as pltpu

M, N = 4096, 1024
BLK = M // 8
STEP = 16

SIZES1 = (16, 32, 16, 64, 128, 256, 512)
SIZES2 = (256, 256)
PATCH_PIECE, PATCH_COLS = 2, 768


def _pieces(sizes):
    return [(sum(sizes[:k]), size) for k, size in enumerate(sizes)]


def _for_rows(start, size, fn):
    if size == STEP:
        fn(start)
        return

    def step(i, carry):
        fn(pl.multiple_of(start + i * STEP, STEP))
        return carry

    lax.fori_loop(0, size // STEP, step, 0)


def _remote(src, dst, peer, send_sem, recv_sem):
    return pltpu.make_async_remote_copy(
        src, dst, send_sem, recv_sem,
        device_id=(peer,), device_id_type=pl.DeviceIdType.MESH,
    )


def _body(t_hbm, out, x, send1, recv1, send2, recv2, last_send, last_recv):
    me = lax.axis_index("i")
    cx = me >> 1
    cy = (me ^ cx) & 1
    odd = (me & 1) == 1

    lanes = (0, 1)
    half = (cx, 1 - cx)
    a = [jnp.where(h == 0, cy, cx) for h in half]
    b = a[::-1]
    peer_a = [me ^ (1 + 2 * h) for h in half]
    peer_b = peer_a[::-1]

    def block(j, far_a, far_b):
        row = (4 * half[j] + 2 * (a[j] ^ far_a) + (b[j] ^ far_b)) * BLK
        return pl.multiple_of(row, BLK)

    def gather(j, far_b, start, size, peer, send_sem, recv_sem):
        rows = out.at[pl.ds(block(j, 0, far_b) + start, size)]
        return _remote(rows, rows, peer, send_sem, recv_sem)

    last = [
        gather(j, 1, 0, BLK, peer_a[j], last_send.at[j], last_recv.at[half[j]])
        for j in lanes
    ]

    def main(go_sem, load_sem, send_sem, recv_sem):
        pieces1, pieces2 = _pieces(SIZES1), _pieces(SIZES2)
        patch_row, patch_rows = pieces1[PATCH_PIECE]
        patch_cols = pl.ds(0, PATCH_COLS)

        x_blocks = ((1, 1), (1, 0), (0, 1), (0, 0))
        loads = [
            [
                pltpu.make_async_copy(
                    t_hbm.at[pl.ds(block(j, *x_blocks[s // BLK]) + s % BLK, n)],
                    x.at[j, pl.ds(s, n)],
                    load_sem.at[2 * k + j],
                )
                for j in lanes
            ]
            for k, (s, n) in enumerate(pieces1 + _pieces((BLK,) * 4)[2:])
        ]

        used = [4]

        def sems():
            used[0] += 2
            k = used[0] - 2
            return [(j, send_sem.at[k + j], recv_sem.at[k + half[j]]) for j in lanes]

        def step1(k, s, n):
            skip = PATCH_COLS if k == PATCH_PIECE else 0
            rows, cols = pl.ds(s, n), pl.ds(skip, N - skip)
            return [
                _remote(send1.at[j, rows, cols], recv1.at[half[j], rows, cols],
                        peer_a[j], send, recv)
                for j, send, recv in sems()
            ]

        def patch(j, row, peer, sem_base):
            return _remote(
                send1.at[j, pl.ds(patch_row, patch_rows), patch_cols],
                recv1.at[half[j], pl.ds(row, patch_rows), patch_cols],
                peer, send_sem.at[j], recv_sem.at[sem_base + half[j]],
            )

        def patch_direct(j):
            return patch(j, patch_row, peer_a[j], 0)

        def patch_around(j):
            return patch(j, 2 * BLK, peer_b[j], 2)

        c1 = [step1(k, s, n) for k, (s, n) in enumerate(pieces1)]
        c2 = [
            [
                _remote(send2.at[j, pl.ds(s, n)], recv2.at[half[j], pl.ds(s, n)],
                        peer_b[j], send, recv)
                for j, send, recv in sems()
            ]
            for s, n in pieces2
        ]
        c3 = [
            [gather(j, 0, s, n, peer_b[j], send, recv) for j, send, recv in sems()]
            for s, n in pieces2
        ]
        c4 = [gather(j, 0, 0, BLK, peer_a[j], send, recv) for j, send, recv in sems()]

        def signal_peers(sem):
            for peer in peer_a:
                pl.semaphore_signal(
                    sem, inc=1, device_id=(peer,), device_id_type=pl.DeviceIdType.MESH
                )

        barrier = pltpu.get_barrier_semaphore()
        pl.when(me != 2)(lambda: signal_peers(barrier))
        for pair in loads:
            for copy in pair:
                copy.start()
        pl.when(odd)(lambda: pl.semaphore_wait(barrier, 1))
        pl.when(~odd)(lambda: pl.semaphore_wait(barrier, 2))
        pl.when(me == 2)(lambda: signal_peers(go_sem))

        for k, (s, n) in enumerate(pieces1):
            for j in lanes:
                loads[k][j].wait()
                if s <= BLK + patch_row < s + n:

                    @pl.when(me == 2)
                    def _(j=j):
                        patch_around(j).wait_recv()
                        got = recv1[half[j], pl.ds(2 * BLK, patch_rows), patch_cols]
                        rows = pl.ds(BLK + patch_row, patch_rows)
                        x[j, rows, patch_cols] += got.astype(jnp.float32)

                def pack(r, j=j):
                    rows = pl.ds(r, STEP)
                    send1[j, rows, :] = x[j, rows, :].astype(jnp.bfloat16)

                _for_rows(s, n, pack)
                if (k, j) == (0, 1):
                    pl.when(~odd)(c1[0][1].start)
                    continue
                c1[k][j].start()
                if (k, j) == (1, 0):

                    @pl.when(odd)
                    def _():
                        pl.semaphore_wait(go_sem, 1)
                        c1[0][1].start()

                if (k, j) == (PATCH_PIECE, 0):
                    pl.when(odd)(patch_around(0).start)
                    pl.when(~odd)(patch_direct(0).start)
                if (k, j) == (PATCH_PIECE, 1):
                    patch_direct(1).start()

        landed = [0]

        def wait_step1(rows):
            while landed[0] < len(pieces1) and pieces1[landed[0]][0] < rows:
                for copy in c1[landed[0]]:
                    copy.wait_recv()
                landed[0] += 1

        wait_step1(patch_row + patch_rows)

        @pl.when(me == 0)
        def _():
            shape = (2, patch_rows, PATCH_COLS)
            rows = pl.ds(patch_row, patch_rows)
            recv1[:, rows, patch_cols] = jnp.zeros(shape, jnp.bfloat16)

        @pl.when(me != 0)
        def _():
            for j in lanes:
                patch_direct(j).wait_recv()

        for copy in loads[-2]:
            copy.wait()
        for k, (s, n) in enumerate(pieces2):
            wait_step1(s + n)
            for j in lanes:

                def add(r, j=j):
                    mine = x[j, pl.ds(2 * BLK + r, STEP), :]
                    near = recv1[half[j], pl.ds(r, STEP), :].astype(jnp.float32)
                    send2[j, pl.ds(r, STEP), :] = (mine + near).astype(jnp.bfloat16)

                _for_rows(s, n, add)
                c2[k][j].start()

        for copy in loads[-1]:
            copy.wait()
        wait_step1(2 * BLK)
        for k, (s, n) in enumerate(pieces2):
            for j in lanes:
                c2[k][j].wait_recv()

                def finish(r, j=j):
                    mine = x[j, pl.ds(3 * BLK + r, STEP), :]
                    near = recv1[half[j], pl.ds(BLK + r, STEP), :].astype(jnp.float32)
                    far = recv2[half[j], pl.ds(r, STEP), :].astype(jnp.float32)
                    v = mine + near + far
                    pos = jnp.maximum(v, 0.0)
                    g = jnp.tanh(v) * v * v + pos * pos * pos
                    row = pl.multiple_of(block(j, 0, 0) + r, STEP)
                    out[pl.ds(row, STEP), :] = g.astype(jnp.bfloat16)

                _for_rows(s, n, finish)
                c3[k][j].start()

        for copy in c4:
            copy.start()
        for pair in c3:
            for copy in pair:
                copy.wait_recv()
        for copy in last:
            copy.start()

        for j in lanes:
            patch_direct(j).wait_send()
        for pair in c1 + c2 + c3:
            for copy in pair:
                copy.wait_send()
        for copy in c4:
            copy.wait()

    n_remote = 4 + 2 * (len(SIZES1) + 2 * len(SIZES2) + 1)
    pl.run_scoped(
        main,
        pltpu.SemaphoreType.REGULAR,
        pltpu.SemaphoreType.DMA((2 * (len(SIZES1) + 2),)),
        pltpu.SemaphoreType.DMA((n_remote,)),
        pltpu.SemaphoreType.DMA((n_remote,)),
    )
    for copy in last:
        copy.wait_send()
    for copy in last:
        copy.wait_recv()


def pallas_dist_f_of_ar_i_m4096_n1024_kernel(t: jax.Array):
    assert t.shape == (M, N)
    return pl.pallas_call(
        _body,
        out_shape=pltpu.VMEM((M, N), jnp.bfloat16),
        in_specs=[pl.BlockSpec(memory_space=pltpu.HBM)],
        out_specs=pl.BlockSpec(memory_space=pltpu.VMEM),
        scratch_shapes=[
            pltpu.VMEM((2, 4 * BLK, N), jnp.float32),
            pltpu.VMEM((2, 2 * BLK, N), jnp.bfloat16),
            pltpu.VMEM((2, 2 * BLK + SIZES1[PATCH_PIECE], N), jnp.bfloat16),
            pltpu.VMEM((2, BLK, N), jnp.bfloat16),
            pltpu.VMEM((2, BLK, N), jnp.bfloat16),
            pltpu.SemaphoreType.DMA((2,)),
            pltpu.SemaphoreType.DMA((2,)),
        ],
        compiler_params=pltpu.CompilerParams(
            collective_id=0, vmem_limit_bytes=48 * 1024 * 1024
        ),
    )(t)
```
